```python
import numpy as np

kernel_name = "dist_sum_ax1_xy_m512_n256"

def setup_inputs():
    return {"x": np.random.randn(1024, 512).astype(np.float32)}

def reference(x: np.ndarray) -> np.ndarray:
    return np.sum(x, axis=1, keepdims=True)
```

```python
import jax
import jax.numpy as jnp
from jax import lax
from jax.experimental import pallas as pl
from jax.experimental.pallas import tpu as pltpu

_LANES = 128
_SUBLANES = 8
_CHUNKS = (224, 192, 96)


def pallas_dist_sum_ax1_xy_m512_n256_kernel(
x: jax.Array,
):
    m, n = x.shape
    assert sum(_CHUNKS) == m and n == 2 * _LANES
    offs = [sum(_CHUNKS[:i]) for i in range(len(_CHUNKS) + 1)]
    groups = m // _LANES
    sends = ((0, groups - 1), (groups - 1, groups))

    def body(x_hbm, o_ref, xbuf, send_buf, recv_buf, ld_sems, send_sems, recv_sems):
        loads = []
        for c, rows in enumerate(_CHUNKS):
            sl = pl.ds(offs[c], rows)
            cp = pltpu.make_async_copy(x_hbm.at[sl], xbuf.at[sl], ld_sems.at[c])
            cp.start()
            loads.append(cp)

        peer = (lax.axis_index("x"), 1 - lax.axis_index("y"))
        barrier = pltpu.get_barrier_semaphore()
        pl.semaphore_signal(barrier, inc=1, device_id=peer,
                            device_id_type=pl.DeviceIdType.MESH)

        lane = lax.broadcasted_iota(jnp.int32, (_SUBLANES, _LANES), 1)
        sub = lax.broadcasted_iota(jnp.int32, (_SUBLANES, _LANES), 0)
        diag = lane - sub

        rdmas = []
        acc = None
        last = None
        for c in range(len(_CHUNKS)):
            loads[c].wait()
            ready = []
            for r0 in range(offs[c], offs[c + 1], _SUBLANES):
                xb = xbuf[pl.ds(r0, _SUBLANES), :]
                col = jnp.sum(xb[:, :_LANES] + xb[:, _LANES:], axis=1, keepdims=True)
                k = r0 % _LANES
                if k == 0:
                    acc = jnp.zeros((_SUBLANES, _LANES), jnp.float32)
                acc = jnp.where(diag == k, col, acc)
                if k == _LANES - _SUBLANES:
                    g = r0 // _LANES
                    last = jnp.sum(acc, axis=0, keepdims=True)
                    send_buf[:, pl.ds(g * _LANES, _LANES)] = last
                    ready += [i for i, (_, g1) in enumerate(sends) if g1 - 1 == g]
            for i in ready:
                if not rdmas:
                    pl.semaphore_wait(barrier, 1)
                g0, g1 = sends[i]
                sl = pl.ds(g0 * _LANES, (g1 - g0) * _LANES)
                rdma = pltpu.make_async_remote_copy(
                    src_ref=send_buf.at[:, sl], dst_ref=recv_buf.at[:, sl],
                    send_sem=send_sems.at[i], recv_sem=recv_sems.at[i],
                    device_id=peer, device_id_type=pl.DeviceIdType.MESH)
                rdma.start()
                rdmas.append(rdma)

        head = pl.ds(0, (groups - 1) * _LANES)
        tail = pl.ds((groups - 1) * _LANES, _LANES)
        rdmas[0].wait_recv()
        o_ref[:, head] = send_buf[:, head] + recv_buf[:, head]
        for rdma in rdmas:
            rdma.wait_send()
        rdmas[1].wait_recv()
        o_ref[:, tail] = last + recv_buf[:, tail]

    out = pl.pallas_call(
        body,
        out_shape=jax.ShapeDtypeStruct((1, m), jnp.float32),
        in_specs=[pl.BlockSpec(memory_space=pl.ANY)],
        out_specs=pl.BlockSpec(memory_space=pltpu.VMEM),
        scratch_shapes=[
            pltpu.VMEM((m, n), jnp.float32),
            pltpu.VMEM((1, m), jnp.float32),
            pltpu.VMEM((1, m), jnp.float32),
            pltpu.SemaphoreType.DMA((len(_CHUNKS),)),
            pltpu.SemaphoreType.DMA((len(sends),)),
            pltpu.SemaphoreType.DMA((len(sends),)),
        ],
        compiler_params=pltpu.CompilerParams(
            collective_id=0, disable_semaphore_checks=True),
    )(x)
    return out.reshape(m, 1)
```

```python
import jax
import jax.numpy as jnp
from jax import lax
from jax.experimental import pallas as pl
from jax.experimental.pallas import tpu as pltpu

_LANES = 128
_SUBLANES = 8

_STAGES = (
    ((480, 32), (0, 208)),
    ((208, 96),),
    ((304, 80),),
    ((384, 96),),
)


def pallas_dist_sum_ax1_xy_m512_n256_kernel(
x: jax.Array,
):
    m, n = x.shape
    pieces = [p for stage in _STAGES for p in stage]
    assert n == 2 * _LANES
    assert sorted(r for s, k in pieces for r in range(s, s + k)) == list(range(m))
    groups = m // _LANES
    head = m - _LANES

    def body(x_hbm, o_ref, *scratch):
        xbufs = scratch[:len(pieces)]
        (send_head, send_tail, recv_head, recv_tail,
         load_sems, send_sems, recv_sems) = scratch[len(pieces):]

        loads = []
        for i, (start, rows) in enumerate(pieces):
            cp = pltpu.make_async_copy(
                x_hbm.at[pl.ds(start, rows)], xbufs[i], load_sems.at[i])
            cp.start(priority=min(i, 1))
            loads.append(cp)

        peer = (lax.axis_index("x"), 1 - lax.axis_index("y"))
        barrier = pltpu.get_barrier_semaphore()
        pl.semaphore_signal(barrier, inc=1, device_id=peer,
                            device_id_type=pl.DeviceIdType.MESH)

        def exchange(i, src, dst):
            return pltpu.make_async_remote_copy(
                src_ref=src, dst_ref=dst,
                send_sem=send_sems.at[i], recv_sem=recv_sems.at[i],
                device_id=peer, device_id_type=pl.DeviceIdType.MESH)

        rdma_head = exchange(0, send_head, recv_head)
        rdma_tail = exchange(1, send_tail, recv_tail)

        lane = lax.broadcasted_iota(jnp.int32, (_SUBLANES, _LANES), 1)
        sub = lax.broadcasted_iota(jnp.int32, (_SUBLANES, _LANES), 0)
        diag = lane - sub

        def fold_sublanes(a):
            rs = [a] + [pltpu.roll(a, _SUBLANES - s, 0) for s in range(1, _SUBLANES)]
            for bit in (1, 2, 4):
                keep = (lane & bit) == 0
                rs = [jnp.where(keep, rs[i], rs[i + 1]) for i in range(0, len(rs), 2)]
            return rs[0][0:1]

        acc = [jnp.zeros((_SUBLANES, _LANES), jnp.float32)] * groups
        left = [_LANES] * groups
        tail = None
        head_sent = False
        i = 0
        for stage in _STAGES:
            for j in range(len(stage)):
                loads[i + j].wait()
            for start, rows in stage:
                for r in range(0, rows, _SUBLANES):
                    xb = xbufs[i][pl.ds(r, _SUBLANES), :]
                    col = jnp.sum(xb[:, :_LANES] + xb[:, _LANES:], axis=1, keepdims=True)
                    g, k = divmod(start + r, _LANES)
                    acc[g] = jnp.where(diag == k, col, acc[g])
                    left[g] -= _SUBLANES
                    if left[g] == 0 and g < groups - 1:
                        send_head[:, pl.ds(g * _LANES, _LANES)] = fold_sublanes(acc[g])
                    elif left[g] == 0:
                        tail = fold_sublanes(acc[g])
                        send_tail[...] = tail
                i += 1
            if not head_sent and not any(left[:-1]):
                pl.semaphore_wait(barrier, 1)
                rdma_head.start()
                head_sent = True
        rdma_tail.start()

        rdma_head.wait_recv()
        o_ref[:, pl.ds(0, head)] = send_head[...] + recv_head[...]
        rdma_head.wait_send()
        rdma_tail.wait_send()
        rdma_tail.wait_recv()
        o_ref[:, pl.ds(head, _LANES)] = tail + recv_tail[...]

    out = pl.pallas_call(
        body,
        out_shape=jax.ShapeDtypeStruct((1, m), jnp.float32),
        in_specs=[pl.BlockSpec(memory_space=pl.ANY)],
        out_specs=pl.BlockSpec(memory_space=pltpu.VMEM),
        scratch_shapes=[pltpu.VMEM((rows, n), jnp.float32) for _, rows in pieces] + [
            pltpu.VMEM((1, head), jnp.float32),
            pltpu.VMEM((1, _LANES), jnp.float32),
            pltpu.VMEM((1, head), jnp.float32),
            pltpu.VMEM((1, _LANES), jnp.float32),
            pltpu.SemaphoreType.DMA((len(pieces),)),
            pltpu.SemaphoreType.DMA((2,)),
            pltpu.SemaphoreType.DMA((2,)),
        ],
        compiler_params=pltpu.CompilerParams(
            collective_id=0, disable_semaphore_checks=True),
    )(x)
    return out.reshape(m, 1)
```

```python
import jax
import jax.numpy as jnp
from jax import lax
from jax.experimental import pallas as pl
from jax.experimental.pallas import tpu as pltpu

_LANES = 128
_SUBLANES = 8

_STAGES = (
    ((480, 32), (0, 208)),
    ((208, 96),),
    ((304, 80),),
    ((384, 96),),
)


def _compiler_params():
    try:
        return pltpu.CompilerParams(collective_id=0, disable_semaphore_checks=True)
    except TypeError:
        return pltpu.CompilerParams(collective_id=0)


def pallas_dist_sum_ax1_xy_m512_n256_kernel(
x: jax.Array,
):
    m, n = x.shape
    pieces = [p for stage in _STAGES for p in stage]
    assert n == 2 * _LANES
    assert sorted(r for s, k in pieces for r in range(s, s + k)) == list(range(m))
    groups = m // _LANES
    head = m - _LANES

    def body(x_hbm, o_ref, *scratch):
        xbufs = scratch[:len(pieces)]
        (send_head, send_tail, recv_head, recv_tail,
         load_sems, send_sems, recv_sems) = scratch[len(pieces):]

        loads = []
        for i, (start, rows) in enumerate(pieces):
            cp = pltpu.make_async_copy(
                x_hbm.at[pl.ds(start, rows)], xbufs[i], load_sems.at[i])
            cp.start(priority=min(i, 1))
            loads.append(cp)

        peer = (lax.axis_index("x"), 1 - lax.axis_index("y"))
        barrier = pltpu.get_barrier_semaphore()
        pl.semaphore_signal(barrier, inc=1, device_id=peer,
                            device_id_type=pl.DeviceIdType.MESH)

        def exchange(i, src, dst):
            return pltpu.make_async_remote_copy(
                src_ref=src, dst_ref=dst,
                send_sem=send_sems.at[i], recv_sem=recv_sems.at[i],
                device_id=peer, device_id_type=pl.DeviceIdType.MESH)

        rdma_head = exchange(0, send_head, recv_head)
        rdma_tail = exchange(1, send_tail, recv_tail)

        lane = lax.broadcasted_iota(jnp.int32, (_SUBLANES, _LANES), 1)
        sub = lax.broadcasted_iota(jnp.int32, (_SUBLANES, _LANES), 0)
        diag = lane - sub

        def fold_sublanes(a):
            rs = [a] + [pltpu.roll(a, _SUBLANES - s, 0) for s in range(1, _SUBLANES)]
            for bit in (1, 2, 4):
                keep = (lane & bit) == 0
                rs = [jnp.where(keep, rs[i], rs[i + 1]) for i in range(0, len(rs), 2)]
            return rs[0][0:1]

        acc = [jnp.zeros((_SUBLANES, _LANES), jnp.float32)] * groups
        left = [_LANES] * groups
        tail = None
        head_sent = False
        i = 0
        for stage in _STAGES:
            for j in range(len(stage)):
                loads[i + j].wait()
            for start, rows in stage:
                for r in range(0, rows, _SUBLANES):
                    xb = xbufs[i][pl.ds(r, _SUBLANES), :]
                    col = jnp.sum(xb[:, :_LANES] + xb[:, _LANES:], axis=1, keepdims=True)
                    g, k = divmod(start + r, _LANES)
                    acc[g] = jnp.where(diag == k, col, acc[g])
                    left[g] -= _SUBLANES
                    if left[g] == 0 and g < groups - 1:
                        send_head[:, pl.ds(g * _LANES, _LANES)] = fold_sublanes(acc[g])
                    elif left[g] == 0:
                        tail = fold_sublanes(acc[g])
                        send_tail[...] = tail
                i += 1
            if not head_sent and not any(left[:-1]):
                pl.semaphore_wait(barrier, 1)
                rdma_head.start()
                head_sent = True
        rdma_tail.start()

        rdma_head.wait_recv()
        o_ref[:, pl.ds(0, head)] = send_head[...] + recv_head[...]
        rdma_head.wait_send()
        rdma_tail.wait_send()
        rdma_tail.wait_recv()
        o_ref[:, pl.ds(head, _LANES)] = tail + recv_tail[...]

    out = pl.pallas_call(
        body,
        out_shape=jax.ShapeDtypeStruct((1, m), jnp.float32),
        in_specs=[pl.BlockSpec(memory_space=pl.ANY)],
        out_specs=pl.BlockSpec(memory_space=pltpu.VMEM),
        scratch_shapes=[pltpu.VMEM((rows, n), jnp.float32) for _, rows in pieces] + [
            pltpu.VMEM((1, head), jnp.float32),
            pltpu.VMEM((1, _LANES), jnp.float32),
            pltpu.VMEM((1, head), jnp.float32),
            pltpu.VMEM((1, _LANES), jnp.float32),
            pltpu.SemaphoreType.DMA((len(pieces),)),
            pltpu.SemaphoreType.DMA((2,)),
            pltpu.SemaphoreType.DMA((2,)),
        ],
        compiler_params=_compiler_params(),
    )(x)
    return out.reshape(m, 1)
```

```python
import jax
import jax.numpy as jnp
from jax import lax
from jax.experimental import pallas as pl
from jax.experimental.pallas import tpu as pltpu

_LANES = 128
_SUBLANES = 8

_STAGES = (
    ((480, 32), (0, 208)),
    ((208, 96),),
    ((304, 80),),
    ((384, 96),),
)


def _compiler_params():
    try:
        return pltpu.CompilerParams(collective_id=0, disable_semaphore_checks=True)
    except TypeError:
        return pltpu.CompilerParams(collective_id=0)


def pallas_dist_sum_ax1_xy_m512_n256_kernel(
x: jax.Array,
):
    m, n = x.shape
    pieces = [p for stage in _STAGES for p in stage]
    assert n == 2 * _LANES
    assert sorted(r for s, k in pieces for r in range(s, s + k)) == list(range(m))
    groups = m // _LANES
    head = m - _LANES

    def body(x_hbm, o_ref, *scratch):
        xbufs = scratch[:len(pieces)]
        (send_head, send_tail, recv_head, recv_tail,
         load_sems, send_sems, recv_sems) = scratch[len(pieces):]

        loads = []
        for i, (start, rows) in enumerate(pieces):
            cp = pltpu.make_async_copy(
                x_hbm.at[pl.ds(start, rows)], xbufs[i], load_sems.at[i])
            cp.start(priority=min(i, 1))
            loads.append(cp)

        peer = (lax.axis_index("x"), 1 - lax.axis_index("y"))
        barrier = pltpu.get_barrier_semaphore()
        pl.semaphore_signal(barrier, inc=1, device_id=peer,
                            device_id_type=pl.DeviceIdType.MESH)

        def exchange(i, src, dst):
            return pltpu.make_async_remote_copy(
                src_ref=src, dst_ref=dst,
                send_sem=send_sems.at[i], recv_sem=recv_sems.at[i],
                device_id=peer, device_id_type=pl.DeviceIdType.MESH)

        rdma_head = exchange(0, send_head, recv_head)
        rdma_tail = exchange(1, send_tail, recv_tail)

        lane = lax.broadcasted_iota(jnp.int32, (_SUBLANES, _LANES), 1)
        sub = lax.broadcasted_iota(jnp.int32, (_SUBLANES, _LANES), 0)
        diag = lane - sub

        def fold_sublanes(a):
            rows = [a[s:s + 1, :] for s in range(_SUBLANES)]
            for bit in (1, 2, 4):
                keep = (lane[0:1, :] & bit) == 0
                rows = [jnp.where(keep, rows[i], rows[i + 1])
                        for i in range(0, len(rows), 2)]
            return rows[0]

        acc = [jnp.zeros((_SUBLANES, _LANES), jnp.float32)] * groups
        left = [_LANES] * groups
        tail = None
        head_sent = False
        i = 0
        for stage in _STAGES:
            for j in range(len(stage)):
                loads[i + j].wait()
            for start, rows in stage:
                for r in range(0, rows, _SUBLANES):
                    xb = xbufs[i][pl.ds(r, _SUBLANES), :]
                    col = jnp.sum(xb[:, :_LANES] + xb[:, _LANES:], axis=1, keepdims=True)
                    g, k = divmod(start + r, _LANES)
                    acc[g] = jnp.where(diag == k, col, acc[g])
                    left[g] -= _SUBLANES
                    if left[g] == 0 and g < groups - 1:
                        send_head[:, pl.ds(g * _LANES, _LANES)] = fold_sublanes(acc[g])
                    elif left[g] == 0:
                        tail = fold_sublanes(acc[g])
                        send_tail[...] = tail
                i += 1
            if not head_sent and not any(left[:-1]):
                pl.semaphore_wait(barrier, 1)
                rdma_head.start()
                head_sent = True
        rdma_tail.start()

        rdma_head.wait_recv()
        o_ref[:, pl.ds(0, head)] = send_head[...] + recv_head[...]
        rdma_head.wait_send()
        rdma_tail.wait_send()
        rdma_tail.wait_recv()
        o_ref[:, pl.ds(head, _LANES)] = tail + recv_tail[...]

    out = pl.pallas_call(
        body,
        out_shape=jax.ShapeDtypeStruct((1, m), jnp.float32),
        in_specs=[pl.BlockSpec(memory_space=pl.ANY)],
        out_specs=pl.BlockSpec(memory_space=pltpu.VMEM),
        scratch_shapes=[pltpu.VMEM((rows, n), jnp.float32) for _, rows in pieces] + [
            pltpu.VMEM((1, head), jnp.float32),
            pltpu.VMEM((1, _LANES), jnp.float32),
            pltpu.VMEM((1, head), jnp.float32),
            pltpu.VMEM((1, _LANES), jnp.float32),
            pltpu.SemaphoreType.DMA((len(pieces),)),
            pltpu.SemaphoreType.DMA((2,)),
            pltpu.SemaphoreType.DMA((2,)),
        ],
        compiler_params=_compiler_params(),
    )(x)
    return out.reshape(m, 1)
```
